```python
import numpy as np

kernel_name = "dist_sparse_attn_localglobal_qseq_kvseq_b2_sq512_skv512_hq8_dh64"

def setup_inputs():
    x = np.random.randn(2, 2048, 768).astype(np.float32)
    Wq = np.random.randn(768, 512).astype(np.float32) * 0.02
    K_ext = np.random.randn(2, 2048, 8, 64).astype(np.float32)
    V_ext = np.random.randn(2, 2048, 8, 64).astype(np.float32)
    Wo = np.random.randn(512, 768).astype(np.float32) * 0.02
    return {"x": x, "Wq": Wq, "K_ext": K_ext, "V_ext": V_ext, "Wo": Wo}

def reference(x, Wq, K_ext, V_ext, Wo):
    B, Sq, Skv, Hq, Dh = 2, 2048, 2048, 8, 64
    Q = (x @ Wq).reshape(B, Sq, Hq, Dh)
    qi = np.arange(Sq)[:, None]
    ki = np.arange(Skv)[None, :]
    local = np.abs(qi - ki) <= 128
    glob = (ki < 32) | (qi < 32)
    mask = local | glob
    scores = np.einsum('bihd,bjhd->bhij', Q, K_ext).astype(np.float32) * 0.125
    scores = np.where(mask[None, None, :, :], scores, -1e9)
    scores_max = scores.max(axis=-1, keepdims=True)
    w = np.exp(scores - scores_max)
    row_keep = mask.any(axis=1)
    w_sum = np.where(row_keep[None, None, :, None], w.sum(axis=-1, keepdims=True), 1.0)
    w = w / w_sum
    w = np.where(row_keep[None, None, :, None], w, 0.0)
    ctx = np.einsum('bhij,bjhd->bihd', w, V_ext).reshape(B, Sq, Hq * Dh)
    return ctx @ Wo
```

```python
import math

import jax
import jax.numpy as jnp
from jax import lax
from jax.experimental import pallas as pl
from jax.experimental.pallas import tpu as pltpu

F32 = jnp.float32
BF16 = jnp.bfloat16
U32 = jnp.uint32

N_DEV = 4
B, S, DM, HD = 2, 512, 768, 512
T = 128
H = T // 2
NP = HD // T
NJ = S // T
NU = B * NP
NG = 32
NEG = -1e30
Q_SCALE = 0.125 * math.log2(math.e)
PART_ROWS = NP * NG // 2 + 8
MAX_LOADS = 22
N_SEMS = 128
NT = (((1,), (1,)), ((), ()))

LOADS = "k0 k1 wq0 xg x00 wq1 x02 e23 x01 x03 wq3 wq2 e45 x12 i2 i3 e67 i45 x11 i67 x13 x10 wo1 wo2 wo0"
WAIT_LAG = dict(e=3, i=3, wo=3, r=3, e0=2, e3=1, e4=4, e5=2, g1=3, gq0=3, gq1=2, gq2=4,
                i6=0, left0=5, r0=0, wo0=0, wq0=2, wq2=3, wq3=3, x03=5, x11=1, xg=4)
Q_OPERANDS = (F32, BF16)
STEPS = """
pe0 send0
pi1 pi0 pe1 gsend0 send1
qp000 gsend1
qp010 qp002 qp012 qk00 sm00 qk02 qsend1
pe3 pe2 gsend2
sm02 qsend0 send2 gsend3 send3
qk12 qp011 qp001 pv00 qp003 qk11 pv02 sm11 qk01 sm12 pv12 qp013 qk03 qp030 qp031 qk10
pv11 qp020 qp023 qp021 qp033 qp022 gs1 pe5 pe4
qsend2 gsend5 qsend3
sm10 sm03 qk13 send5
sm01 sm13 send4 gsend4
pv01 pv10 qp032 qp122 qp132 qp102 qp112 pi2 pv03 qk22 qk20 pv13 pi3 sm22 qk21 qk23 pe6
pe7 pv22 sm20 qk31 qk30 gs0 gsend7 send6
sm21 gsend6
sm30 send7
gs2 pv20 pv30 go0 go1 pv21 qk33 pi5 qk32 sm31 qp111 qp131 sm33 sm32 sm23 qp121 pi4 qk52
pv32 pv23 gs4 pv31 pv33 pi7 go2 pi6 qp101 qk51 gs5 gs3 sm51 qp123 gs6 gs7 qp103 qp113
qp100 go5 qp130 go3 qp120 qp133 go7 go4 qp110 go6
rsend0 rsend1
qk40 wo1 out031 pv51 qk42 qk72 qk43 wo2 sm52 sm43 out021 qk41 pv43 sm41 out032 out022
pv52 qk61 wo0 sm42 qk62 out020 sm62 pv41 sm72 out010 pv42 qk50 qk71 pv72 sm61 sm40 pv62
qk63 sm71 out011 sm63 pv71 qk60 pv61 out122 out030 sm60 qk53 pv40 qk70 out120 sm50 out111
qk73 out121 out012 sm53 sm73 pv63 pv73 pv50 sm70 pv53 merge0 out112 pv60 pv70 out130 out132
out001 merge1 out131 out000 out101 out110 out002 out100 out102
"""


def _pack(v):
    return pltpu.bitcast(v, U32)


def _unpack(v):
    return pltpu.bitcast(v, BF16)


def _col_max(v):
    return jnp.max(v.reshape(-1, 8, T), axis=0)


def _col_sum(v):
    return jnp.sum(v.reshape(-1, 8, T), axis=0)


def _body(x_hbm, wq_hbm, k_hbm, v_hbm, wo_hbm, out_ref,
          xf, xg, wqf, wof, kf, vf, wo16, kv, gkv, gq, q16, ctx, part, dma_sems, entry_sem):
    me = lax.axis_index("i")
    is_first = me == 0
    has_left = me > 0
    has_right = me < N_DEV - 1

    sem_ids = {}

    def sem(*key, count=1, pick=0):
        if key not in sem_ids:
            sem_ids[key] = sem_ids.get("used", 0)
            sem_ids["used"] = sem_ids[key] + count
            assert sem_ids["used"] <= N_SEMS
        return dma_sems.at[sem_ids[key] + pick]

    def remote(src, dst, send_sem, recv_sem, device):
        return pltpu.make_async_remote_copy(
            src, dst, send_sem, recv_sem,
            device_id=(device,), device_id_type=pl.DeviceIdType.MESH)

    def arrival(expected, buf, *key, count=1, pick=0):
        def wait(shift):
            copy = pltpu.make_async_copy(buf, buf, sem(*key, count=count, pick=pick + shift))
            if expected is True:
                copy.wait()
            else:
                pl.when(expected)(copy.wait)
        return wait

    pending = {}
    queue, started = [], []
    for name in LOADS.split():
        kind = name.rstrip("0123456789")
        ids = [int(c) for c in name[len(kind):]]
        if kind in ("k", "e", "i"):
            b, p = divmod(ids[0], NP)
            cols = dict(k=[(0, S)], e=[(0, T), (S - T, T)], i=[(T, S - 2 * T)])[kind]
            cuts = [(b, pl.ds(p * T, len(ids) * T), pl.ds(*c)) for c in cols]
            pairs = [(s.at[c], d.at[c]) for c in cuts for s, d in ((k_hbm, kf), (v_hbm, vf))]
            names = [f"{k}{u}" for u in ids for k in ("ei" if kind == "k" else kind)]
        elif kind == "xg":
            pairs, names = [(x_hbm.at[1, pl.ds(0, NG)], xg)], [name]
        elif kind == "x":
            c = (ids[0], pl.ds(ids[1] * T, (len(ids) - 1) * T))
            pairs, names = [(x_hbm.at[c], xf.at[c])], [f"x{ids[0]}{j}" for j in ids[1:]]
        elif kind == "wq":
            c = (slice(None), pl.ds(ids[0] * T, len(ids) * T))
            pairs, names = [(wq_hbm.at[c], wqf.at[c])], [f"wq{p}" for p in ids]
        else:
            c = (slice(None), pl.ds(ids[0] * 2 * T, len(ids) * 2 * T))
            pairs, names = [(wo_hbm.at[c], wof.at[c])], [f"wo{n}" for n in ids]
        waits = []
        for src, dst in pairs:
            queue.append((waits, pltpu.make_async_copy(src, dst, sem(name, len(waits)))))
            waits.append(arrival(True, dst, name, len(waits)))
        pending.update({n: waits for n in names})

    def start_loads(limit=MAX_LOADS):
        while queue and sum(bool(waits) for waits in started) < limit:
            waits, copy = queue.pop(0)
            copy.start()
            started.append(waits)

    start_loads(2)
    barrier = pltpu.get_barrier_semaphore()
    left = lax.rem(me + N_DEV - 1, N_DEV)
    right = lax.rem(me + 1, N_DEV)
    for neighbour in (left, right):
        pl.semaphore_signal(barrier, inc=1, device_id=(neighbour,),
                            device_id_type=pl.DeviceIdType.MESH)
    start_loads()

    def neighbours_entered(_):
        pl.semaphore_wait(barrier, 2)
        for d in (0, 2):
            pl.when(me == 3)(lambda: pl.semaphore_signal(
                entry_sem, inc=1, device_id=(d,), device_id_type=pl.DeviceIdType.MESH))

    def all_entered(_):
        pl.when((me & 1) == 0)(lambda: pl.semaphore_wait(entry_sem, 1))

    pending["neighbours"] = [neighbours_entered]
    pending["everyone"] = [all_entered]
    for u in range(NU):
        pending[f"left{u}"] = [arrival(has_left, kv.at[u, 0], "from left", u)]
        pending[f"right{u}"] = [arrival(has_right, kv.at[u, NJ + 1], "from right", u)]
        pending[f"g{u}"] = [arrival(has_left, gkv.at[1, u], "g in", u)]
    for p in range(NP):
        pending[f"gq{p}"] = [arrival(has_left, gq.at[1, p], "q in", p)]
    for b in range(B):
        pending[f"r{b}"] = [
            arrival(is_first, part.at[b, 1 + i], "r in", b, count=N_DEV - 1, pick=i)
            for i in range(N_DEV - 1)]

    results = []

    def need(name):
        waits = pending.pop(name, [])
        assert all(waits is not w for w, _ in queue), name
        shift = 0
        lag = WAIT_LAG.get(name, WAIT_LAG.get(name.rstrip("0123456789"), 0))
        if waits and len(results) >= lag > 0:
            shift = jnp.where(results[-lag][0, 0] < 0, me >> 2, 0)
        while waits:
            waits.pop(0)(shift)
            shift = 0

    lane = lax.broadcasted_iota(jnp.int32, (1, T), 1)
    low = lane < H
    row = lax.broadcasted_iota(jnp.int32, (H, T), 0)
    col = lax.broadcasted_iota(jnp.int32, (H, T), 1)
    d_az = row - col
    d_za = row - (col ^ H)
    d_half = row - (col & (H - 1))
    big = jnp.int32(4 * T)

    slots = [jnp.where(has_left, 0, 1), *range(1, NJ + 1), jnp.where(has_right, NJ + 1, NJ)]
    g_slot = jnp.where(is_first, 0, 1)

    def halo_copies(u):
        return ((has_left, remote(kv.at[u, 1], kv.at[u, NJ + 1],
                                  sem("to left", u), sem("from right", u), left)),
                (has_right, remote(kv.at[u, NJ], kv.at[u, 0],
                                   sem("to right", u), sem("from left", u), right)))

    def g_copy(u, d):
        return remote(gkv.at[0, u], gkv.at[1, u], sem("g out", u, d), sem("g in", u), d)

    def q_copy(p, d):
        return remote(gq.at[0, p], gq.at[1, p], sem("q out", p, d), sem("q in", p), d)

    def r_copy(b):
        slot = jnp.maximum(me - 1, 0)
        return remote(part.at[b, 0], part.at[b, 1 + slot], sem("r out", b),
                      sem("r in", b, count=N_DEV - 1, pick=slot), 0)

    def send(u):
        need("neighbours")
        for exists, copy in halo_copies(u):
            pl.when(exists)(copy.start)

    held = []

    def spread(copy_to):
        need("neighbours")
        for d in range(1, N_DEV):
            if d == 2 and "everyone" in pending:
                held.append(copy_to(d))
            else:
                pl.when(is_first)(copy_to(d).start)

    def gsend(u):
        spread(lambda d: g_copy(u, d))

    def qsend(p):
        spread(lambda d: q_copy(p, d))

    def rsend(b):
        need("neighbours")
        need("everyone")
        pl.when(has_left)(r_copy(b).start)

    live = {}

    def prepare(u, blocks):
        b, p = divmod(u, NP)
        for j in blocks:
            c = (b, pl.ds(p * T, T), pl.ds(j * T, T))
            keys = _pack(kf[c].astype(BF16).T)
            vals = vf[c].astype(BF16)
            kv[u, 1 + j, 0] = keys
            kv[u, 1 + j, 1] = _pack(vals)
            if j == 0:
                gkv[0, u, pl.ds(0, NG // 2)] = keys[:NG // 2]
                gkv[0, u, pl.ds(NG // 2, NG // 2)] = _pack(vals.T)[:NG // 2]

    def pe(u):
        need(f"e{u}")
        prepare(u, (0, NJ - 1))

    def pi(u):
        need(f"i{u}")
        prepare(u, range(1, NJ - 1))

    def qp(b, p, j):
        need(f"wq{p}")
        need(f"x{b}{j}")
        skip = NG if (b, j) == (1, 0) else 0
        rows = xf[b, pl.ds(j * T + skip, T - skip)]
        first = (b, j) == (0, 0)
        if first:
            need("xg")
            rows = jnp.concatenate([rows, xg[...]], axis=0)
        q = jnp.dot(rows.astype(Q_OPERANDS[b]), wqf[:, pl.ds(p * T, T)].astype(Q_OPERANDS[b]),
                    preferred_element_type=F32)
        results.append(q[:8])
        q = _pack((q * Q_SCALE).astype(BF16))
        q16[b * NP + p, j, pl.ds(skip // 2, H - skip // 2)] = q[:H - skip // 2]
        if first:
            gq[0, p, 0] = q[:NG // 2]
            gq[0, p, 1] = q[H:]
            q16[NP + p, 0, pl.ds(0, NG // 2)] = q[H:]

    def qk(u, j):
        need(f"g{u}")
        if j == 0:
            need(f"left{u}")
        if j == NJ - 1:
            need(f"right{u}")
        q = q16[u, j]
        zero = jnp.zeros_like(q)
        q0 = jnp.where(low, q, zero)
        q1 = jnp.where(low, zero, q)
        a, z = slice(0, H // 2), slice(H // 2, H)

        def scores(keys, queries):
            return lax.dot_general(_unpack(keys), _unpack(queries), NT, preferred_element_type=F32)

        before, own, after = slots[j:j + 3]
        mid = jnp.concatenate([kv[u, before, 0, z], kv[u, own, 0], kv[u, after, 0, a],
                               gkv[g_slot, u, pl.ds(0, NG // 2)]], axis=0)
        s0 = scores(mid, q0)
        sa = scores(kv[u, before, 0, a], jnp.concatenate([q0[a], q1[a]], axis=0))
        s1 = scores(mid, jnp.concatenate([q1[z], q1[a]], axis=0))
        sz = scores(kv[u, after, 0, z], jnp.concatenate([q1[z], q0[z]], axis=0))
        results.append(s0[H:H + 8])
        lo = jnp.where(is_first, big, 0) if j == 0 else 0
        hi = jnp.where(has_right, 0, -big) if j == NJ - 1 else 0

        def mask(s, d):
            glob = s[4 * H:]
            if j < 2:
                outside = d[:NG] < jnp.where(is_first, -big if j == 0 else 0, big)
                glob = jnp.where(outside, glob, NEG)
            return jnp.concatenate([jnp.where(d >= lo - H, s[:H], NEG), s[H:3 * H],
                                    jnp.where(d <= hi, s[3 * H:4 * H], NEG), glob], axis=0)

        s0, s1 = mask(s0, d_az), mask(s1, d_za)
        sa = jnp.where(d_half >= lo, sa, NEG)
        sz = jnp.where(d_half <= hi, sz, NEG)
        live["s", u, j] = s0, s1, sa, sz

    def sm(u, j):
        s0, s1, sa, sz = live.pop(("s", u, j))
        ma, mz = _col_max(sa), _col_max(sz)
        m0 = jnp.max(jnp.maximum(_col_max(s0), jnp.where(low, ma, mz)), axis=0, keepdims=True)
        m1 = jnp.max(jnp.maximum(_col_max(s1), jnp.where(low, mz, ma)), axis=0, keepdims=True)

        def weights(s, m):
            e = jnp.exp2(s - m)
            return e, _col_sum(e)

        pa, la = weights(sa, jnp.where(low, m0, m1))
        pz, lz = weights(sz, jnp.where(low, m1, m0))
        p0, l0 = weights(s0, m0)
        p1, l1 = weights(s1, m1)
        l0 = jnp.sum(l0 + jnp.where(low, la, lz), axis=0, keepdims=True)
        l1 = jnp.sum(l1 + jnp.where(low, lz, la), axis=0, keepdims=True)
        zero = jnp.zeros_like(pa)
        p0 = jnp.concatenate([jnp.where(low, pa, zero), p0[:2 * T],
                              jnp.where(low, zero, pz), p0[2 * T:]], axis=0)
        p1 = jnp.concatenate([jnp.where(low, zero, pa), p1[:2 * T],
                              jnp.where(low, pz, zero), p1[2 * T:]], axis=0)
        live["p", u, j] = (p0.astype(BF16), 1.0 / l0), (p1.astype(BF16), 1.0 / l1)

    def pv(u, j):
        b, p = divmod(u, NP)
        if ("vg", u) not in live:
            live["vg", u] = _unpack(gkv[g_slot, u, pl.ds(NG // 2, NG // 2)]).T
        outs = []
        for h, (w, inv) in enumerate(live.pop(("p", u, j))):
            dims = pl.ds(h * H // 2, H // 2)
            vals = _unpack(jnp.concatenate([kv[u, i, 1, dims] for i in slots[j:j + 3]], axis=1))
            vals = jnp.concatenate([vals, live["vg", u][h * H:(h + 1) * H]], axis=1)
            outs.append(jnp.dot(vals, w, preferred_element_type=F32) * inv)
        results.append(outs[0][:8])
        t = _pack(jnp.concatenate(outs, axis=0).astype(BF16).T)
        a, z = t[:H // 2], t[H // 2:]
        ctx[b, j, :, pl.ds(p * T, T)] = jnp.concatenate(
            [jnp.where(low, a, z), jnp.where(low, z, a)], axis=0)

    def gs(u):
        b, p = divmod(u, NP)
        need(f"gq{p}")
        q = gq[g_slot, p, b]
        zero = jnp.zeros_like(q)
        q = jnp.concatenate([jnp.where(low, q, zero), jnp.where(low, zero, q)], axis=0)
        keys = jnp.concatenate([kv[u, 1 + j, 0] for j in range(NJ)], axis=0)
        live["g", u] = lax.dot_general(_unpack(q), _unpack(keys), NT, preferred_element_type=F32)

    def go(u):
        b, p = divmod(u, NP)
        s = live.pop(("g", u))
        m = jnp.max(s, axis=1, keepdims=True)
        e = jnp.exp2(s - m)
        l = jnp.sum(e, axis=1, keepdims=True)
        vals = _unpack(jnp.concatenate([kv[u, 1 + j, 1] for j in range(NJ)], axis=1))
        o = lax.dot_general(e.astype(BF16), vals, NT, preferred_element_type=F32) * (1.0 / l)
        part[b, 0, pl.ds(p * NG // 2, NG // 2)] = _pack(
            jnp.where(low, o[:NG], o[NG:]).astype(BF16))
        lse = m + jnp.log2(l)
        stats, done = live.pop(("stats", b), (jnp.zeros((8, T), F32), 0))
        for i in range(8):
            stats = jnp.where((lane >> 2) == 8 * p + i, lse[8 * i:8 * i + 8], stats)
        if done + 1 < NP:
            live["stats", b] = stats, done + 1
        else:
            part[b, 0, pl.ds(NP * NG // 2, 8)] = pltpu.bitcast(stats, U32)

    def merge(b):
        need(f"r{b}")
        parts = [part.at[b, jnp.where(is_first, d, 0) if d else 0] for d in range(N_DEV)]
        lse = [pltpu.bitcast(r[pl.ds(NP * NG // 2, 8)], F32) for r in parts]
        top = jnp.maximum(jnp.maximum(lse[0], lse[1]), jnp.maximum(lse[2], lse[3]))
        w = [jnp.exp2(v - top) for v in lse]
        inv = 1.0 / (w[0] + w[1] + w[2] + w[3])
        w = jnp.concatenate([v * inv for v in w], axis=0)
        for p in range(NP):
            cols = [w[:, 4 * (8 * p + i):4 * (8 * p + i) + 1] for i in range(8)]
            scales = [jnp.where(low, cols[i], cols[4 + i]) for i in range(4)]
            acc = 0.0
            for d, r in enumerate(parts):
                scale = jnp.concatenate([v[8 * d:8 * d + 8] for v in scales], axis=0)
                acc += scale * _unpack(r[pl.ds(p * NG // 2, NG // 2)]).astype(F32)
            c = (b, 0, pl.ds(0, NG // 2), pl.ds(p * T, T))
            ctx[c] = jnp.where(is_first, _pack(acc.astype(BF16)), ctx[c])

    def wo(n):
        need(f"wo{n}")
        w = wof[:, pl.ds(n * 2 * T, 2 * T)]
        b11, b12, b21, b22 = w[:2 * T, :T], w[:2 * T, T:], w[2 * T:, :T], w[2 * T:, T:]
        for i, v in enumerate((b11 + b22, b11, b12 - b22, b21 - b11, b22, b11 + b12, b21 + b22)):
            wo16[n, i] = _pack(v.astype(BF16))

    def out(b, j, n):
        if ("a", b, j) not in live:
            quads = [_unpack(ctx[b, j, pl.ds(r, H // 2), pl.ds(k, 2 * T)])
                     for r in (0, H // 2) for k in (0, 2 * T)]
            a11, a12, a21, a22 = (v.astype(F32) for v in quads)
            live["a", b, j] = [v.astype(BF16) for v in (
                a11 + a22, a21 + a22, quads[0], quads[3], a11 + a12, a21 - a11, a12 - a22)]
        m = [jnp.dot(v, _unpack(wo16[n, i]), preferred_element_type=F32)
             for i, v in enumerate(live["a", b, j])]
        o = jnp.concatenate([
            jnp.concatenate([m[0] + m[3] - m[4] + m[6], m[2] + m[4]], axis=1),
            jnp.concatenate([m[1] + m[3], m[0] - m[1] + m[2] + m[5]], axis=1)], axis=0)
        results.append(o[:8, :T])
        out_ref[b, pl.ds(j * T, T), pl.ds(n * 2 * T, 2 * T)] = o

    steps = dict(send=send, gsend=gsend, qsend=qsend, rsend=rsend, pe=pe, pi=pi, qp=qp, qk=qk,
                 sm=sm, pv=pv, gs=gs, go=go, merge=merge, wo=wo, out=out)
    for line in STEPS.strip().splitlines():
        for step in line.split():
            name = step.rstrip("0123456789")
            if "send" in name:
                results.clear()
            steps[name](*(int(c) for c in step[len(name):]))
        if "send" in name:
            if held:
                need("everyone")
            while held:
                pl.when(is_first)(held.pop(0).start)
            start_loads()
    assert not pending, pending

    for u in range(NU):
        for exists, copy in halo_copies(u):
            pl.when(exists)(copy.wait_send)
        for d in range(1, N_DEV):
            pl.when(is_first)(g_copy(u, d).wait_send)
    for d in range(1, N_DEV):
        for p in range(NP):
            pl.when(is_first)(q_copy(p, d).wait_send)
    for b in range(B):
        pl.when(has_left)(r_copy(b).wait_send)


def pallas_dist_sparse_attn_localglobal_qseq_kvseq_b2_sq512_skv512_hq8_dh64_kernel(
    x: jax.Array,
    Wq: jax.Array,
    K_ext: jax.Array,
    V_ext: jax.Array,
    Wo: jax.Array,
):
    kt = K_ext.transpose(0, 2, 3, 1).reshape(B, HD, S)
    vt = V_ext.transpose(0, 2, 3, 1).reshape(B, HD, S)
    return pl.pallas_call(
        _body,
        out_shape=jax.ShapeDtypeStruct((B, S, DM), F32),
        in_specs=[pl.BlockSpec(memory_space=pltpu.MemorySpace.HBM)] * 5,
        out_specs=pl.BlockSpec(memory_space=pltpu.VMEM),
        scratch_shapes=[
            pltpu.VMEM((B, S, DM), F32),
            pltpu.VMEM((NG, DM), F32),
            pltpu.VMEM((DM, HD), F32),
            pltpu.VMEM((HD, DM), F32),
            pltpu.VMEM((B, HD, S), F32),
            pltpu.VMEM((B, HD, S), F32),
            pltpu.VMEM((DM // (2 * T), 7, T, T), U32),
            pltpu.VMEM((NU, NJ + 2, 2, H, T), U32),
            pltpu.VMEM((2, NU, NG, T), U32),
            pltpu.VMEM((2, NP, B, NG // 2, T), U32),
            pltpu.VMEM((NU, NJ, H, T), U32),
            pltpu.VMEM((B, NJ, H, HD), U32),
            pltpu.VMEM((B, N_DEV, PART_ROWS, T), U32),
            pltpu.SemaphoreType.DMA((N_SEMS,)),
            pltpu.SemaphoreType.REGULAR,
        ],
        compiler_params=pltpu.CompilerParams(
            collective_id=0,
            vmem_limit_bytes=48 * 2**20,
            flags={"XLA_TPU_RESCHEDULE_DMA_DONES": True},
            disable_semaphore_checks=True,
        ),
    )(x, Wq, kt, vt, Wo)
```
